```python
import numpy as np

kernel_name = "dist_rs_then_ag_i_m2048_n1024"

def setup_inputs():
    return {"x": np.random.randn(8192, 1024).astype(np.float32)}

def reference(x: np.ndarray) -> np.ndarray:
    return x.reshape(4, 2048, 1024).sum(axis=0)
```

```python
import jax
import jax.numpy as jnp
from jax import lax
from jax.experimental import pallas as pl
from jax.experimental.pallas import tpu as pltpu

M, N = 2048, 1024
Q = M // 4
TILE = 16


def _pieces(sizes):
    assert sum(sizes) == Q
    return [(sum(sizes[:k]), n) for k, n in enumerate(sizes)]


C1 = _pieces((16, 48, 64, 128, 256))
C2 = _pieces((256, 256))
C3 = _pieces((256, 256))


def _body(x_hbm, out, xs, xo, s1, r1, s2, r2, ld_s, ld_o, s1s, s1r, s2s, s2r, s3s, s3r):
    me = lax.axis_index("i")
    partner = (me ^ 1, me ^ 3)
    own = ((me ^ (me >> 1)) & 1, (me >> 1) & 1)
    mine = [pl.multiple_of((2 * s + own[s]) * Q, Q) for s in range(2)]
    theirs = [pl.multiple_of((2 * s + 1 - own[s]) * Q, Q) for s in range(2)]
    mesh = pl.DeviceIdType.MESH

    def load_theirs(s, k):
        r, n = C1[k]
        return pltpu.make_async_copy(
            x_hbm.at[pl.ds(theirs[s] + r, n)], xs.at[s, pl.ds(r, n)], ld_s.at[s, k])

    def load_mine(s, k):
        r, n = C2[k]
        return pltpu.make_async_copy(
            x_hbm.at[pl.ds(mine[s] + r, n)], xo.at[s, pl.ds(r, n)], ld_o.at[s, k])

    def phase1(s, k):
        rows = pl.ds(*C1[k])
        return pltpu.make_async_remote_copy(
            s1.at[s, rows], r1.at[s, rows], s1s.at[s, k], s1r.at[s, k],
            device_id=(partner[s],), device_id_type=mesh)

    def phase2(s, k):
        rows = pl.ds(*C2[k])
        return pltpu.make_async_remote_copy(
            s2.at[s, rows], r2.at[s, rows], s2s.at[s, k], s2r.at[s, k],
            device_id=(partner[1 - s],), device_id_type=mesh)

    def phase3(s, k, base):
        r, n = C3[k]
        rows = out.at[pl.ds(base[s] + r, n)]
        return pltpu.make_async_remote_copy(
            rows, rows, s3s.at[s, k], s3r.at[s, k],
            device_id=(partner[s],), device_id_type=mesh)

    def for_tiles(n, f):
        if n == TILE:
            f(0)
        else:
            pl.loop(0, n // TILE)(lambda i: f(pl.multiple_of(i * TILE, TILE)))

    for s in range(2):
        load_theirs(s, 0).start()
    barrier = pltpu.get_barrier_semaphore()
    for s in range(2):
        pl.semaphore_signal(barrier, inc=1, device_id=(partner[s],), device_id_type=mesh)
    for k in range(1, len(C1)):
        for s in range(2):
            load_theirs(s, k).start()
    for k in range(len(C2)):
        for s in range(2):
            load_mine(s, k).start()

    for k, (r, n) in enumerate(C1):
        for s in range(2):
            load_theirs(s, k).wait()

            def round_tile(i, s=s, r=r):
                rows = pl.ds(r + i, TILE)
                s1[s, rows, :] = xs[s, rows, :].astype(jnp.bfloat16)

            for_tiles(n, round_tile)
            if k > 0:
                phase1(s, k).start()
        if k == 0:
            pl.semaphore_wait(barrier, 2)
            for s in range(2):
                phase1(s, k).start()

    landed = 0
    for k, (r, n) in enumerate(C2):
        needed = [j for j in range(landed, len(C1)) if C1[j][0] < r + n]
        for s in range(2):
            for j in needed:
                phase1(s, j).wait_recv()
            load_mine(s, k).wait()

            def pair_sum(i, s=s, r=r):
                rows = pl.ds(r + i, TILE)
                total = xo[s, rows, :] + r1[s, rows, :].astype(jnp.float32)
                s2[s, rows, :] = total.astype(jnp.bfloat16)

            for_tiles(n, pair_sum)
            phase2(s, k).start()
        landed += len(needed)

    landed = 0
    for k, (r, n) in enumerate(C3):
        needed = [j for j in range(landed, len(C2)) if C2[j][0] < r + n]
        for s in range(2):
            for j in needed:
                phase2(s, j).wait_recv()

            def full_sum(i, s=s, r=r):
                rows = pl.ds(r + i, TILE)
                total = (s2[s, rows, :].astype(jnp.float32)
                         + r2[s, rows, :].astype(jnp.float32))
                out[pl.ds(mine[s] + r + i, TILE), :] = total.astype(jnp.bfloat16)

            for_tiles(n, full_sum)
            phase3(s, k, mine).start()
        landed += len(needed)

    for s in range(2):
        for k in range(len(C1)):
            phase1(s, k).wait_send()
        for k in range(len(C2)):
            phase2(s, k).wait_send()
    for k in range(len(C3)):
        for s in range(2):
            phase3(s, k, mine).wait_send()
            phase3(s, k, theirs).wait_recv()


def pallas_dist_rs_then_ag_i_m2048_n1024_kernel(x: jax.Array):
    dma = pltpu.SemaphoreType.DMA
    out = pl.pallas_call(
        _body,
        out_shape=pltpu.VMEM((M, N), jnp.bfloat16),
        in_specs=[pl.BlockSpec(memory_space=pl.ANY)],
        out_specs=pl.BlockSpec(memory_space=pltpu.VMEM),
        scratch_shapes=[
            pltpu.VMEM((2, Q, N), jnp.float32),
            pltpu.VMEM((2, Q, N), jnp.float32),
            pltpu.VMEM((2, Q, N), jnp.bfloat16),
            pltpu.VMEM((2, Q, N), jnp.bfloat16),
            pltpu.VMEM((2, Q, N), jnp.bfloat16),
            pltpu.VMEM((2, Q, N), jnp.bfloat16),
            dma((2, len(C1))), dma((2, len(C2))),
            dma((2, len(C1))), dma((2, len(C1))),
            dma((2, len(C2))), dma((2, len(C2))),
            dma((2, len(C3))), dma((2, len(C3))),
        ],
        compiler_params=pltpu.CompilerParams(
            collective_id=0, vmem_limit_bytes=48 * 2**20),
    )(x)
    return out.astype(jnp.float32)
```

```python
import jax
import jax.numpy as jnp
from jax import lax
from jax.experimental import pallas as pl
from jax.experimental.pallas import tpu as pltpu

M, N = 2048, 1024
ROWS = M // 8
TILE = 16
VREG = (8, 128)
WORDS = 4 * ROWS // TILE
PLANES = WORDS // 8
STREAM = WORDS // 4
HEAD = WORDS + PLANES + STREAM - 1
REST = (HEAD + 1, 2 * WORDS - HEAD)
ZERO_AT = 39

COPIES = {
    "a": ((0, 4), (4, 8), (12, 12), (24, 16), (40, 24), (64, 24)),
    "b": ((0, 32), (32, 56)),
    "c": ((64, 24), (0, 32), (32, 32)),
    "d": ((0, 32), (32, 32), (64, 24)),
    "e": ((0, 88),),
    "f": ((36, 52), (4, 32), (0, 4)),
}
SLOT = {name: i for i, name in enumerate("abcdef")}
REST_COPY = len(COPIES["a"])

I32 = jnp.int32
srl = lax.shift_right_logical


def _each(byte):
    value = byte * 0x01010101
    return value - (1 << 32) if value >= 1 << 31 else value


def _spread(byte):
    byte = byte | (byte << 8)
    return byte | (byte << 16)


def _widen(flags):
    return (flags - srl(flags, 7)) | flags


def _swap(a, b):
    t = ((a << 7) ^ b) & 0x7F807F80
    return a ^ srl(t, 7), b ^ t


def _lengths(depth, low):
    q = srl(depth, 1) & _each(0x1F)
    inside = q + _each(0x80 - 1)
    swapped = inside & ~((q + _each(0x80 - 3)) | (low << 7)) & _each(0x80)
    above = ~inside & _each(0x80)
    return ((q ^ (srl(swapped, 7) | srl(swapped, 6)))
            + (srl(above, 4) - srl(above, 7))
            + (srl(q + _each(0x80 - 7), 7) & _each(1)))


def _depths(length, low):
    beyond = length + _each(0x80 - 8)
    swapped = ~((length + _each(0x80 - 3)) | (low << 7)) & _each(0x80)
    above = ((length + _each(0x80 - 7)) ^ beyond) & _each(0x80)
    q = ((length ^ (srl(swapped, 7) | srl(swapped, 6)))
         - (srl(above, 4) - srl(above, 7))
         - (srl(beyond, 7) & _each(1)))
    return (q << 1) | low


def _encode_exponents(exps, tx, slot):
    total = 0
    for k in range(0, WORDS, 8):
        e = exps[:, k]
        total = total + (e & 0x00FF00FF) + (srl(e, 8) & 0x00FF00FF)
    total = ((total & 0xFFFF) + srl(total, 16)).astype(jnp.float32)
    total = jnp.sum(jnp.sum(total, axis=2, keepdims=True), axis=1, keepdims=True)
    top = jnp.clip(srl(total.astype(I32) + 9 * 2**14, 15), ZERO_AT, 255)
    top = jnp.broadcast_to(top, (2, *VREG))
    tops = _spread(top)
    zero, one = jnp.zeros_like(top), jnp.ones_like(top)

    def segment(j, carry):
        pos, pending, deep, long, wide, stream = carry
        stream = [*stream, zero]
        plane, mark = zero, pos
        for z in range(8):
            e = exps[:, 8 * j + z]
            depth = tops - e
            nonzero = ((e & _each(0x7F)) + _each(0x7F)) | e
            deep = deep | (((depth + _each(0x80 - ZERO_AT)) | depth) & nonzero)
            depth = depth - (_widen(~nonzero & _each(0x80)) & (tops - _each(ZERO_AT)))
            low = depth & _each(1)
            plane = (plane << 1) | low
            end = _lengths(depth, low) - 1
            end = end + (end << 8)
            end = end + (end << 16)
            long = long | end
            last = srl(end, 24)
            codes = ((one << (end & 31)) | (one << (srl(end, 8) & 31))
                     | (one << (srl(end, 16) & 31)) | (one << (last & 31)))
            word, bit = srl(pos, 5), pos & 31
            filled = pending | (codes << bit)
            stream = [jnp.where(word == k, filled, v) for k, v in enumerate(stream)]
            pos = pos + last + 1
            pending = jnp.where(srl(pos, 5) != word, srl(srl(codes, 1), bit ^ 31), filled)
            if z % 4 == 3:
                wide, mark = wide | (pos - mark - 1), pos
        tx[:, slot, WORDS + j] = plane
        tx[:, slot, WORDS + PLANES + j] = stream[0]
        return pos - 32, pending, deep, long, wide, tuple(stream[1:])

    pos, pending, deep, long, wide, stream = lax.fori_loop(
        0, PLANES, segment, (zero, zero, zero, zero, zero, (zero,) * 8))
    stream = [jnp.where(srl(pos, 5) == k, pending, v) for k, v in enumerate(stream)]
    corner = ((lax.broadcasted_iota(I32, top.shape, 1) == 0)
              & (lax.broadcasted_iota(I32, top.shape, 2) == 0))
    for k in range(7):
        tx[:, slot, HEAD - 7 + k] = stream[k]
    tx[:, slot, HEAD] = jnp.where(corner, stream[7] | (top << 16), stream[7])

    misfit = ((pos > jnp.where(corner, 256 - 16, 256))
              | (((deep & _each(0x80)) | srl(long, 29) | srl(wide, 6)) != 0))
    misfit = jnp.where(misfit, 1.0, 0.0)
    uncoded = [jnp.max(misfit[s]) > 0.5 for s in range(2)]
    for s in range(2):
        @pl.when(uncoded[s])
        def _():
            tx[s, slot, pl.ds(WORDS, HEAD - WORDS)] = exps[s, pl.ds(0, HEAD - WORDS)]
            tx[s, slot, HEAD] = jnp.full(VREG, 1 << 24, I32)
            tx[s, slot, pl.ds(*REST)] = exps[s, pl.ds(HEAD - WORDS, REST[1])]
    return uncoded


def _header(rx, s, slot):
    return srl(rx[s, slot, HEAD][0, 0], 16)


def _decode_exponents(rx, slot, uncoded, exps):
    tops = _spread(jnp.stack([jnp.full(VREG, _header(rx, s, slot), I32) for s in range(2)]))

    def segment(j, pos):
        stream = [rx[:, slot, WORDS + PLANES + jnp.minimum(j + k, STREAM - 1)] for k in range(11)]
        plane = rx[:, slot, WORDS + j]
        for z in range(8):
            if z % 4 == 0:
                near = stream
                for hop, keep in ((4, 6), (2, 4), (1, 3)):
                    skip = (pos & (32 * hop)) != 0
                    near = [jnp.where(skip, near[k + hop], near[k]) for k in range(keep)]
                near = [jnp.where(pos >= 256, stream[8 + k], near[k]) for k in range(3)]
                bit = pos & 31
                lo, hi = (srl(near[k], bit) | ((near[k + 1] << 1) << (bit ^ 31)) for k in range(2))
            bits, end = lo, 0
            for k in range(4):
                rest = bits & (bits - 1)
                f = lax.bitcast_convert_type((bits ^ rest).astype(jnp.float32), I32)
                f = srl(f, 23 - 8 * k) & (0xFF << 8 * k) if k < 3 else (f << 1) & -(1 << 24)
                bits, end = rest, end | f
            end = end - _each(127)
            last = srl(end, 24)
            pos = pos + last + 1
            if z % 4 != 3:
                last = last & 31
                lo, hi = srl(srl(lo, 1), last) | (hi << (last ^ 31)), srl(srl(hi, 1), last)
            depth = _depths(end - (end << 8) + 1, srl(plane, 7 - z) & _each(1))
            is_zero = ~((depth ^ _each(ZERO_AT)) + _each(0x7F)) & _each(0x80)
            exps[:, slot, 8 * j + z] = (tops - depth) & ~_widen(is_zero)
        return pos - 32

    lax.fori_loop(0, PLANES, segment, jnp.zeros_like(tops))
    for s in range(2):
        @pl.when(uncoded[s])
        def _():
            exps[s, slot, pl.ds(0, HEAD - WORDS)] = rx[s, slot, pl.ds(WORDS, HEAD - WORDS)]
            exps[s, slot, pl.ds(HEAD - WORDS, REST[1])] = rx[s, slot, pl.ds(*REST)]


def _body(x_hbm, out, xs, tx, rx, tx_exps, rx_exps, load_sem, tx_sem, rx_sem, ready):
    me = lax.axis_index("i")
    mesh = pl.DeviceIdType.MESH

    def near(s):
        return me ^ (1 + 2 * s)

    def far(s):
        return me ^ (3 - 2 * s)

    def rows(s, chip, first, count):
        return pl.ds(pl.multiple_of(s * (M // 2) + chip * ROWS + first, TILE), count)

    def load(s, name, k=0):
        first, count = (w // 4 * TILE for w in (COPIES["a"][k] if name == "a" else (0, WORDS)))
        chip = {"a": me ^ 2, "b": near(s), "c": far(s), "d": me}[name]
        return pltpu.make_async_copy(
            x_hbm.at[rows(s, chip, first, count)], xs.at[s, SLOT[name], pl.ds(first, count)],
            load_sem.at[s, 3 + k if k else SLOT[name]])

    def copy(s, name, k):
        words = pl.ds(*(REST if k == REST_COPY else COPIES[name][k]))
        src = rx.at[s, SLOT["d"]] if name == "f" else tx.at[s, min(SLOT[name], SLOT["d"])]
        return pltpu.make_async_remote_copy(
            src.at[words], rx.at[s, SLOT[name], words],
            tx_sem.at[s, SLOT[name], k], rx_sem.at[s, SLOT[name], k],
            device_id=(far(s) if name in "cd" else near(s),), device_id_type=mesh)

    def for_tiles(words, step):
        first, count = words[0] // 4, min(words[1], WORDS - words[0]) // 4
        group = 2 if count % 2 == 0 else 1
        if count <= 2:
            for t in range(count):
                step(first + t)
        else:
            @pl.loop(0, count // group)
            def _(i):
                for t in range(group):
                    step(first + group * i + t)

    def split(name, words, values, streams=(0, 1)):
        def step(t):
            for s in streams:
                w = pltpu.bitcast(values(s, t), I32)
                for q in range(4):
                    a, b = w[:, 256 * q:256 * q + 128], w[:, 256 * q + 128:256 * q + 256]
                    e, sm = _swap((a << 1) | srl(a, 31), b)
                    tx_exps[s, 4 * t + q] = e
                    tx[s, SLOT[name], 4 * t + q] = sm
        for_tiles(words, step)

    def join(s, name, t):
        columns = []
        for q in range(4):
            a, b = _swap(rx_exps[s, SLOT[name], 4 * t + q], rx[s, SLOT[name], 4 * t + q])
            columns += [srl(a, 1) | (a << 31), b]
        return pltpu.bitcast(jnp.concatenate(columns, axis=1), jnp.bfloat16)

    def own(s, name, t):
        return xs[s, SLOT[name], pl.ds(pl.multiple_of(t * TILE, TILE), TILE), :]

    def rounded(name):
        return lambda s, t: own(s, name, t).astype(jnp.bfloat16)

    def pair_sum(s, t):
        return (own(s, "c", t) + join(s, "a", t).astype(jnp.float32)).astype(jnp.bfloat16)

    def total(s, t):
        v = (own(s, "d", t) + join(s, "b", t).astype(jnp.float32)
             + join(s, "c", t).astype(jnp.float32)).astype(jnp.bfloat16)
        out[rows(s, me, t * TILE, TILE), :] = v
        return v

    def store(name, chip, words):
        def step(t):
            for s in range(2):
                out[rows(s, chip(s), t * TILE, TILE), :] = join(s, name, t)
        for_tiles(words, step)

    sent_uncoded = {}

    def send(name, k, uncoded=None):
        for s in range(2):
            copy(s, name, k).start()
        if uncoded is not None:
            sent_uncoded[name] = uncoded
            for s in range(2):
                @pl.when(uncoded[s])
                def _():
                    copy(s, name, REST_COPY).start()

    def receive(name, ks=None):
        for k in range(len(COPIES[name])) if ks is None else ks:
            for s in range(2):
                copy(s, name, k).wait_recv()

    def receive_rest(name):
        uncoded = [_header(rx, s, SLOT[name]) > 255 for s in range(2)]
        for s in range(2):
            @pl.when(uncoded[s])
            def _():
                copy(s, name, REST_COPY).wait_recv()
        return uncoded

    def encode(name):
        return _encode_exponents(tx_exps, tx, SLOT[name])

    def decode(name, uncoded):
        _decode_exponents(rx, SLOT[name], uncoded, rx_exps)

    def drain(name):
        for s in range(2):
            for k in range(len(COPIES[name])):
                copy(s, name, k).wait_send()

            @pl.when(sent_uncoded[name][s])
            def _():
                copy(s, name, REST_COPY).wait_send()

    def signal(sem, chip):
        pl.semaphore_signal(sem, inc=1, device_id=(chip,), device_id_type=mesh)

    lead = me >> 1
    other = 1 - lead
    load(lead, "a", 0).start()
    load(lead, "a", 1).start()
    barrier = pltpu.get_barrier_semaphore()

    @pl.when(me == 0)
    def _():
        signal(barrier, 1)
        signal(barrier, 3)

    @pl.when((me & 1) == 1)
    def _():
        signal(barrier, 2)
        pl.semaphore_wait(barrier, 1)
        signal(ready.at[lead], 0)

    @pl.when(me == 2)
    def _():
        pl.semaphore_wait(barrier, 2)
        signal(ready.at[1], 1)
        signal(ready.at[0], 3)

    pieces = len(COPIES["a"]) - 1
    load(other, "a", 0).start()
    load(other, "a", 1).start()
    for k in range(2, pieces):
        for s in range(2):
            load(s, "a", k).start()

    for s, waits in ((lead, me == 0), (other, me != 2)):
        for k in range(2):
            load(s, "a", k).wait()
            split("a", COPIES["a"][k], rounded("a"), (s,))
            if k == 0:
                @pl.when(waits)
                def _():
                    pl.semaphore_wait(ready.at[s], 1)
            copy(s, "a", k).start()
    for k in range(2, pieces):
        if k == pieces - 1:
            for s in range(2):
                load(s, "b").start()
        for s in range(2):
            load(s, "a", k).wait()
        split("a", COPIES["a"][k], rounded("a"))
        send("a", k)
    for name in "cd":
        for s in range(2):
            load(s, name).start()
    send("a", pieces, encode("a"))

    for s in range(2):
        load(s, "b").wait()
    split("b", (0, WORDS), rounded("b"))
    send("b", 0)
    send("b", 1, encode("b"))

    receive("a")
    for s in range(2):
        load(s, "c").wait()
    decode("a", receive_rest("a"))
    split("c", (0, WORDS), pair_sum)
    send("c", 0, encode("c"))
    send("c", 1)
    send("c", 2)

    receive("b")
    for s in range(2):
        load(s, "d").wait()
    decode("b", receive_rest("b"))
    receive("c", [0])
    decode("c", receive_rest("c"))

    for k in range(2):
        receive("c", [k + 1])
        split("d", COPIES["d"][k], total)
        send("d", k)
    uncoded = encode("d")
    send("d", 2, uncoded)
    send("e", 0, uncoded)

    receive("d")
    uncoded = receive_rest("d")
    send("f", 0, uncoded)
    send("f", 1)
    send("f", 2)
    decode("d", uncoded)
    store("d", far, (0, WORDS))

    receive("e")
    decode("e", receive_rest("e"))
    store("e", near, (0, WORDS))

    for name in "abcde":
        drain(name)
    for k, words in enumerate(COPIES["f"]):
        receive("f", [k])
        if k == 0:
            decode("f", receive_rest("f"))
        store("f", lambda s: me ^ 2, words)
    drain("f")


def pallas_dist_rs_then_ag_i_m2048_n1024_kernel(x: jax.Array):
    dma = pltpu.SemaphoreType.DMA
    return pl.pallas_call(
        _body,
        out_shape=pltpu.VMEM((M, N), jnp.bfloat16),
        in_specs=[pl.BlockSpec(memory_space=pl.ANY)],
        out_specs=pl.BlockSpec(memory_space=pltpu.VMEM),
        scratch_shapes=[
            pltpu.VMEM((2, 4, ROWS, N), jnp.float32),
            pltpu.VMEM((2, 4, 2 * WORDS + 1, *VREG), I32),
            pltpu.VMEM((2, 6, 2 * WORDS + 1, *VREG), I32),
            pltpu.VMEM((2, WORDS, *VREG), I32),
            pltpu.VMEM((2, 6, WORDS, *VREG), I32),
            dma((2, 2 + REST_COPY)),
            dma((2, 6, REST_COPY + 1)),
            dma((2, 6, REST_COPY + 1)),
            pltpu.SemaphoreType.REGULAR((2,)),
        ],
        compiler_params=pltpu.CompilerParams(
            collective_id=0, vmem_limit_bytes=48 * 2**20, disable_semaphore_checks=True),
    )(x)
```

```python
import functools

import jax
import jax.numpy as jnp
from jax import lax
from jax.experimental import pallas as pl
from jax.experimental.pallas import tpu as pltpu

M, N = 2048, 1024
ROWS = M // 8
TILE = 16
VREG = (8, 128)
WORDS = 4 * ROWS // TILE
PLANES = WORDS // 8
STREAM = WORDS // 4
HEAD = WORDS + PLANES + STREAM - 2
HEAD_ROWS = 5
UNCODED = 1 << 15
REST = (HEAD + 1, 2 * WORDS - HEAD)
ZERO_AT = 39

COPIES = {
    "a": ((0, 4), (4, 8), (12, 12), (24, 16), (40, 24), (64, 23)),
    "b": ((0, 32), (32, 55)),
    "c": ((64, 23), (0, 32), (32, 32)),
    "d": ((0, 32), (32, 32), (64, 23)),
    "e": ((0, 87),),
    "f": ((36, 51), (4, 32), (0, 4)),
}
SLOT = {name: i for i, name in enumerate("abcdef")}
REST_COPY = len(COPIES["a"])

I32 = jnp.int32
srl = lax.shift_right_logical


def _words(first, count=1):
    if isinstance(first, int):
        short = VREG[0] - HEAD_ROWS if first + count == HEAD + 1 else 0
        return pl.ds(VREG[0] * first, VREG[0] * count - short)
    return pl.ds(pl.multiple_of(VREG[0] * first, VREG[0]), VREG[0] * count)


def _each(byte):
    value = byte * 0x01010101
    return value - (1 << 32) if value >= 1 << 31 else value


def _spread(byte):
    byte = byte | (byte << 8)
    return byte | (byte << 16)


def _widen(flags):
    return (flags - srl(flags, 7)) | flags


def _swap(a, b):
    t = ((a << 7) ^ b) & 0x7F807F80
    return a ^ srl(t, 7), b ^ t


def _lengths(depth, low):
    q = srl(depth, 1) & _each(0x1F)
    inside = q + _each(0x80 - 1)
    swapped = inside & ~((q + _each(0x80 - 3)) | (low << 7)) & _each(0x80)
    above = ~inside & _each(0x80)
    return ((q ^ (srl(swapped, 7) | srl(swapped, 6)))
            + (srl(above, 5) | srl(above, 6))
            + (srl(q + _each(0x80 - 6), 7) & _each(1)))


def _depths(length, low):
    beyond = length + _each(0x80 - 7)
    swapped = ~((length + _each(0x80 - 3)) | (low << 7)) & _each(0x80)
    above = ((length + _each(0x80 - 6)) ^ beyond) & _each(0x80)
    q = ((length ^ (srl(swapped, 7) | srl(swapped, 6)))
         - (srl(above, 5) | srl(above, 6))
         - (srl(beyond, 7) & _each(1)))
    return (q << 1) | low


def _sum(v):
    total = jnp.sum(jnp.sum(v.astype(jnp.float32), axis=-2, keepdims=True), axis=-1, keepdims=True)
    return jnp.broadcast_to(total.astype(I32), v.shape)


def _offset(sample):
    mean = srl(_sum((sample & 0x7FFF) + (srl(sample, 16) & 0x7FFF)), 11)
    offset = (61 - mean) & 127
    return offset | (offset << 16)


def _encode_exponents(exps, offsets, tx, slot):
    total = 0
    for k in range(0, WORDS, 8):
        e = exps[:, _words(k)]
        total = total + (e & 0x00FF00FF) + (srl(e, 8) & 0x00FF00FF)
    total = _sum((total & 0xFFFF) + srl(total, 16))
    top = jnp.clip(srl(total + 9 * 2**14, 15), ZERO_AT, 255)
    tops = _spread(top)
    zero, one = jnp.zeros_like(top), jnp.ones_like(top)

    def segment(j, carry):
        pos, pending, deep, long, wide, stream = carry
        stream = [*stream, zero]
        plane, mark = zero, pos
        for z in range(8):
            e = exps[:, _words(8 * j + z)]
            depth = tops - e
            nonzero = ((e & _each(0x7F)) + _each(0x7F)) | e
            deep = deep | (((depth + _each(0x80 - ZERO_AT)) | depth) & nonzero)
            depth = depth - (_widen(~nonzero & _each(0x80)) & (tops - _each(ZERO_AT)))
            low = depth & _each(1)
            plane = (plane << 1) | low
            end = _lengths(depth, low) - 1
            end = end + (end << 8)
            end = end + (end << 16)
            long = long | end
            last = srl(end, 24)
            codes = ((one << (end & 31)) | (one << (srl(end, 8) & 31))
                     | (one << (srl(end, 16) & 31)) | (one << (last & 31)))
            word, bit = srl(pos, 5), pos & 31
            filled = pending | (codes << bit)
            stream = [jnp.where(word == k, filled, v) for k, v in enumerate(stream)]
            pos = pos + last + 1
            pending = jnp.where(srl(pos, 5) != word, srl(srl(codes, 1), bit ^ 31), filled)
            if z % 4 == 3:
                wide, mark = wide | (pos - mark - 1), pos
        tx[:, slot, _words(WORDS + j)] = plane
        tx[:, slot, _words(WORDS + PLANES + j)] = stream[0]
        return pos - 32, pending, deep, long, wide, tuple(stream[1:])

    pos, pending, deep, long, wide, stream = lax.fori_loop(
        0, PLANES, segment, (zero, zero, zero, zero, zero, (zero,) * 8))
    stream = [jnp.where(srl(pos, 5) == k, pending, v) for k, v in enumerate(stream)]
    for k in range(6):
        tx[:, slot, _words(HEAD - 6 + k)] = stream[k]

    row = lax.broadcasted_iota(I32, top.shape, 1)
    info = top | ((offsets[...] & 127) << 8)
    head, left = info, stream[6:]
    for k in range(1, HEAD_ROWS):
        source = jnp.where(left[1] != 0, row + 8, jnp.where(left[0] != 0, row, 0))
        source = jnp.max(source.astype(jnp.float32), axis=1, keepdims=True).astype(I32)
        kept = [jnp.where(row + 8 * i == source, v, 0) for i, v in enumerate(left)]
        left = [v ^ w for v, w in zip(left, kept)]
        kept = kept[0] | kept[1]
        kept = functools.reduce(jnp.bitwise_or, [kept[:, r:r + 1] for r in range(VREG[0])])
        head = jnp.where(row == k, kept, jnp.where(row == 0, head | (source << 12 + 4 * k), head))
    tx[:, slot, _words(HEAD)] = head[:, :HEAD_ROWS]

    misfit = (deep & _each(0x80)) | srl(long, 29) | srl(wide, 6) | left[0] | left[1]
    misfit = (misfit != 0) | (pos > 256)
    misfit = jnp.where(misfit, 1.0, 0.0)
    uncoded = [jnp.max(misfit[s]) > 0.5 for s in range(2)]
    for s in range(2):
        @pl.when(uncoded[s])
        def _():
            tx[s, slot, _words(WORDS, HEAD - WORDS)] = exps[s, _words(0, HEAD - WORDS)]
            tx[s, slot, _words(HEAD)] = info[s, :HEAD_ROWS] | UNCODED
            tx[s, slot, _words(*REST)] = exps[s, _words(HEAD - WORDS, REST[1])]
    return uncoded


def _decode_exponents(rx, slot, uncoded, exps):
    head = rx[:, slot, _words(HEAD)]
    info = jnp.broadcast_to(head[:, :1], (2, *VREG))
    tops = _spread(info & 0xFF)
    row = lax.broadcasted_iota(I32, tops.shape, 1)
    ends = [0, 0]
    for k in range(1, HEAD_ROWS):
        source = srl(info, 12 + 4 * k) & 15
        ends = [v | jnp.where(row + 8 * i == source, head[:, k:k + 1], 0) for i, v in enumerate(ends)]

    def segment(j, pos):
        stream = [rx[:, slot, _words(WORDS + PLANES + jnp.minimum(j + k, STREAM - 3))]
                  for k in range(11)]
        for i, v in enumerate(ends):
            stream[7:] = [jnp.where(j + k == STREAM - 2 + i, v, stream[k]) for k in range(7, 11)]
        plane = rx[:, slot, _words(WORDS + j)]
        for z in range(8):
            if z % 4 == 0:
                near = stream
                for hop, keep in ((4, 6), (2, 4), (1, 3)):
                    skip = (pos & (32 * hop)) != 0
                    near = [jnp.where(skip, near[k + hop], near[k]) for k in range(keep)]
                near = [jnp.where(pos >= 256, stream[8 + k], near[k]) for k in range(3)]
                bit = pos & 31
                lo, hi = (srl(near[k], bit) | ((near[k + 1] << 1) << (bit ^ 31)) for k in range(2))
            bits, end = lo, 0
            for k in range(4):
                rest = bits & (bits - 1)
                f = lax.bitcast_convert_type((bits ^ rest).astype(jnp.float32), I32)
                f = srl(f, 23 - 8 * k) & (0xFF << 8 * k) if k < 3 else (f << 1) & -(1 << 24)
                bits, end = rest, end | f
            end = end - _each(127)
            last = srl(end, 24)
            pos = pos + last + 1
            if z % 4 != 3:
                last = last & 31
                lo, hi = srl(srl(lo, 1), last) | (hi << (last ^ 31)), srl(srl(hi, 1), last)
            depth = _depths(end - (end << 8) + 1, srl(plane, 7 - z) & _each(1))
            is_zero = ~((depth ^ _each(ZERO_AT)) + _each(0x7F)) & _each(0x80)
            exps[:, slot, _words(8 * j + z)] = (tops - depth) & ~_widen(is_zero)
        return pos - 32

    lax.fori_loop(0, PLANES, segment, jnp.zeros_like(tops))
    for s in range(2):
        @pl.when(uncoded[s])
        def _():
            exps[s, slot, _words(0, HEAD - WORDS)] = rx[s, slot, _words(WORDS, HEAD - WORDS)]
            exps[s, slot, _words(HEAD - WORDS, REST[1])] = rx[s, slot, _words(*REST)]
    offsets = srl(info, 8) & 127
    return offsets | (offsets << 16)


def _body(x_hbm, out, xs, tx, rx, tx_exps, rx_exps, tx_offsets, load_sem, tx_sem, rx_sem, ready):
    me = lax.axis_index("i")
    mesh = pl.DeviceIdType.MESH

    def near(s):
        return me ^ (1 + 2 * s)

    def far(s):
        return me ^ (3 - 2 * s)

    def rows(s, chip, first, count):
        return pl.ds(pl.multiple_of(s * (M // 2) + chip * ROWS + first, TILE), count)

    def load(s, name, k=0):
        first, count = (w // 4 * TILE for w in (COPIES["a"][k] if name == "a" else (0, WORDS)))
        chip = {"a": me ^ 2, "b": near(s), "c": far(s), "d": me}[name]
        return pltpu.make_async_copy(
            x_hbm.at[rows(s, chip, first, count)], xs.at[s, SLOT[name], pl.ds(first, count)],
            load_sem.at[s, 3 + k if k else SLOT[name]])

    def copy(s, name, k):
        words = _words(*(REST if k == REST_COPY else COPIES[name][k]))
        src = rx.at[s, SLOT["d"]] if name == "f" else tx.at[s, min(SLOT[name], SLOT["d"])]
        return pltpu.make_async_remote_copy(
            src.at[words], rx.at[s, SLOT[name], words],
            tx_sem.at[s, SLOT[name], k], rx_sem.at[s, SLOT[name], k],
            device_id=(far(s) if name in "cd" else near(s),), device_id_type=mesh)

    def for_tiles(words, step):
        first, count = words[0] // 4, min(words[1], WORDS - words[0]) // 4
        group = 2 if count % 2 == 0 else 1
        if count <= 2:
            for t in range(count):
                step(first + t)
        else:
            @pl.loop(0, count // group)
            def _(i):
                for t in range(group):
                    step(first + group * i + t)

    def split(name, words, values, streams=(0, 1)):
        plain = 4 if name == "a" else 0
        if words[0] == plain:
            for s in streams:
                tx_offsets[s] = _offset(pltpu.bitcast(values(s, 0), I32)[:, :VREG[1]])
        offsets = [tx_offsets[s] if words[0] >= plain else 0 for s in streams]

        def step(t):
            for s, offset in zip(streams, offsets):
                w = pltpu.bitcast(values(s, t), I32)
                for q in range(4):
                    a, b = (w[:, c:c + 128] + offset for c in (256 * q, 256 * q + 128))
                    e, sm = _swap((a << 1) | srl(a, 31), b)
                    tx_exps[s, _words(4 * t + q)] = e
                    tx[s, SLOT[name], _words(4 * t + q)] = sm
        for_tiles(words, step)

    def join(s, name, t):
        columns, offset = [], rx_offsets[name][s]
        if name == "a":
            offset = jnp.where(t == 0, 0, offset)
        for q in range(4):
            word = _words(4 * t + q)
            a, b = _swap(rx_exps[s, SLOT[name], word], rx[s, SLOT[name], word])
            columns += [(srl(a, 1) | (a << 31)) - offset, b - offset]
        return pltpu.bitcast(jnp.concatenate(columns, axis=1), jnp.bfloat16)

    def own(s, name, t):
        return xs[s, SLOT[name], pl.ds(pl.multiple_of(t * TILE, TILE), TILE), :]

    def rounded(name):
        return lambda s, t: own(s, name, t).astype(jnp.bfloat16)

    def pair_sum(s, t):
        return (own(s, "c", t) + join(s, "a", t).astype(jnp.float32)).astype(jnp.bfloat16)

    def total(s, t):
        v = (own(s, "d", t) + join(s, "b", t).astype(jnp.float32)
             + join(s, "c", t).astype(jnp.float32)).astype(jnp.bfloat16)
        out[rows(s, me, t * TILE, TILE), :] = v
        return v

    def store(name, chip, words):
        def step(t):
            for s in range(2):
                out[rows(s, chip(s), t * TILE, TILE), :] = join(s, name, t)
        for_tiles(words, step)

    rx_offsets, sent_uncoded = {}, {}

    def send(name, k, uncoded=None):
        for s in range(2):
            copy(s, name, k).start()
        if uncoded is not None:
            sent_uncoded[name] = uncoded
            for s in range(2):
                @pl.when(uncoded[s])
                def _():
                    copy(s, name, REST_COPY).start()

    def receive(name, ks=None):
        for k in range(len(COPIES[name])) if ks is None else ks:
            for s in range(2):
                copy(s, name, k).wait_recv()

    def receive_rest(name):
        uncoded = [(rx[s, SLOT[name], _words(HEAD)][0, 0] & UNCODED) != 0 for s in range(2)]
        for s in range(2):
            @pl.when(uncoded[s])
            def _():
                copy(s, name, REST_COPY).wait_recv()
        return uncoded

    def encode(name):
        return _encode_exponents(tx_exps, tx_offsets, tx, SLOT[name])

    def decode(name, uncoded):
        rx_offsets[name] = _decode_exponents(rx, SLOT[name], uncoded, rx_exps)

    def drain(name):
        for s in range(2):
            for k in range(len(COPIES[name])):
                copy(s, name, k).wait_send()

            @pl.when(sent_uncoded[name][s])
            def _():
                copy(s, name, REST_COPY).wait_send()

    def signal(sem, chip):
        pl.semaphore_signal(sem, inc=1, device_id=(chip,), device_id_type=mesh)

    lead = me >> 1
    other = 1 - lead
    load(lead, "a", 0).start()
    load(lead, "a", 1).start()
    barrier = pltpu.get_barrier_semaphore()

    @pl.when(me == 0)
    def _():
        signal(barrier, 1)
        signal(barrier, 3)

    @pl.when((me & 1) == 1)
    def _():
        signal(barrier, 2)
        pl.semaphore_wait(barrier, 1)
        signal(ready.at[lead], 0)

    @pl.when(me == 2)
    def _():
        pl.semaphore_wait(barrier, 2)
        signal(ready.at[1], 1)
        signal(ready.at[0], 3)

    pieces = len(COPIES["a"]) - 1
    load(other, "a", 0).start()
    load(other, "a", 1).start()
    for k in range(2, pieces):
        for s in range(2):
            load(s, "a", k).start()

    for s, waits in ((lead, me == 0), (other, me != 2)):
        for k in range(2):
            load(s, "a", k).wait()
            split("a", COPIES["a"][k], rounded("a"), (s,))
            if k == 0:
                @pl.when(waits)
                def _():
                    pl.semaphore_wait(ready.at[s], 1)
            copy(s, "a", k).start()
    for k in range(2, pieces):
        if k == pieces - 1:
            for s in range(2):
                load(s, "b").start()
        for s in range(2):
            load(s, "a", k).wait()
        split("a", COPIES["a"][k], rounded("a"))
        send("a", k)
    for name in "cd":
        for s in range(2):
            load(s, name).start()
    send("a", pieces, encode("a"))

    for s in range(2):
        load(s, "b").wait()
    split("b", (0, WORDS), rounded("b"))
    send("b", 0)
    send("b", 1, encode("b"))

    receive("a")
    for s in range(2):
        load(s, "c").wait()
    decode("a", receive_rest("a"))
    split("c", (0, WORDS), pair_sum)
    send("c", 0, encode("c"))
    send("c", 1)
    send("c", 2)

    receive("b")
    for s in range(2):
        load(s, "d").wait()
    decode("b", receive_rest("b"))
    receive("c", [0])
    decode("c", receive_rest("c"))

    for k in range(2):
        receive("c", [k + 1])
        split("d", COPIES["d"][k], total)
        send("d", k)
    uncoded = encode("d")
    send("d", 2, uncoded)
    send("e", 0, uncoded)

    receive("d")
    uncoded = receive_rest("d")
    send("f", 0, uncoded)
    send("f", 1)
    send("f", 2)
    decode("d", uncoded)
    store("d", far, (0, WORDS))

    receive("e")
    decode("e", receive_rest("e"))
    store("e", near, (0, WORDS))

    for name in "abcde":
        drain(name)
    for k, words in enumerate(COPIES["f"]):
        receive("f", [k])
        if k == 0:
            decode("f", receive_rest("f"))
        store("f", lambda s: me ^ 2, words)
    drain("f")


def pallas_dist_rs_then_ag_i_m2048_n1024_kernel(x: jax.Array):
    dma = pltpu.SemaphoreType.DMA
    return pl.pallas_call(
        _body,
        out_shape=pltpu.VMEM((M, N), jnp.bfloat16),
        in_specs=[pl.BlockSpec(memory_space=pl.ANY)],
        out_specs=pl.BlockSpec(memory_space=pltpu.VMEM),
        scratch_shapes=[
            pltpu.VMEM((2, 4, ROWS, N), jnp.float32),
            pltpu.VMEM((2, 4, (2 * WORDS + 1) * VREG[0], VREG[1]), I32),
            pltpu.VMEM((2, 6, (2 * WORDS + 1) * VREG[0], VREG[1]), I32),
            pltpu.VMEM((2, WORDS * VREG[0], VREG[1]), I32),
            pltpu.VMEM((2, 6, WORDS * VREG[0], VREG[1]), I32),
            pltpu.VMEM((2, *VREG), I32),
            dma((2, 2 + REST_COPY)),
            dma((2, 6, REST_COPY + 1)),
            dma((2, 6, REST_COPY + 1)),
            pltpu.SemaphoreType.REGULAR((2,)),
        ],
        compiler_params=pltpu.CompilerParams(
            collective_id=0, vmem_limit_bytes=48 * 2**20, disable_semaphore_checks=True),
    )(x)
```
